```python
import numpy as np

kernel_name = "dist_moe_shared_ep_outshard_n256_d128_e2_h256"

def setup_inputs():
    x = np.random.randn(256, 128).astype(np.float32)
    router_W = np.random.randn(128, 8).astype(np.float32) * 0.1
    scores64 = x.astype(np.float64) @ router_W.astype(np.float64)
    route_idx = np.argsort(-scores64, axis=-1)[:, :1].astype(np.int32)
    expert_W = np.random.randn(8, 128, 256).astype(np.float32) * 0.02
    shared_W = np.random.randn(128, 256).astype(np.float32) * 0.02
    return {"x": x, "router_W": router_W, "route_idx": route_idx, "expert_W": expert_W, "shared_W": shared_W}

def reference(x, router_W, route_idx, expert_W, shared_W):
    scores = x @ router_W
    s_max = scores.max(axis=-1, keepdims=True)
    probs = np.exp(scores - s_max)
    probs = probs / probs.sum(axis=-1, keepdims=True)
    shared = x @ shared_W
    out = np.zeros((256, 256), dtype=np.float32)
    for i in range(256):
        e = int(route_idx[i, 0])
        out[i] = shared[i] + probs[i, e] * (x[i] @ expert_W[e])
    return out
```

```python
import functools
import jax, jax.numpy as jnp
from jax import lax
from jax.experimental import pallas as pl
from jax.experimental.pallas import tpu as pltpu

NDEV, M, D, H, EL = 4, 64, 128, 256, 2
N = NDEV * M
MESH = pl.DeviceIdType.MESH
f32, bf16, u32, i32 = jnp.float32, jnp.bfloat16, jnp.uint32, jnp.int32
NT = (((1,), (1,)), ((), ()))

def _pack(y):
    lo = lax.bitcast_convert_type(y[:, :128].astype(bf16).astype(f32), u32)
    hi = lax.bitcast_convert_type(y[:, 128:].astype(bf16).astype(f32), u32)
    return (lo >> 16) | hi

def make(order="i,w0,x,w1", split=1, fused=False, trace=False, selfmm="with", logical=False):
  def kern(x, router_W, route_idx, expert_W, shared_W):
    def body(x_h, rt_h, idx_h, w_h, s_h, o_ref):
        def scoped(xv, wv, sv, rtv, iv, sbuf, rbuf, lsem, ssem, rsem, done):
            def mark(name):
                if trace:
                    with jax.named_scope(name):
                        pl.delay(1)
            me = lax.axis_index("i")
            KS = (2, 1, 3, 0)
            peer = [(me + k) & 3 for k in KS]
            blk = lambda s: pl.ds(pl.multiple_of(peer[s] * M, M), M)
            cp = dict(
                w0=pltpu.make_async_copy(w_h.at[0], wv.at[0], lsem.at[0]),
                x=pltpu.make_async_copy(x_h.at[blk(0)], xv.at[pl.ds(0, M)], lsem.at[0]),
                w1=pltpu.make_async_copy(w_h.at[1], wv.at[1], lsem.at[1]),
                i=pltpu.make_async_copy(idx_h, iv, lsem.at[2]))
            for k in order.split(","):
                cp[k].start()
            bar = pltpu.get_barrier_semaphore()
            for s in range(3):
                pl.semaphore_signal(bar, inc=1, device_id=(peer[s],), device_id_type=MESH)
            rest = [pltpu.make_async_copy(x_h.at[blk(s)], xv.at[pl.ds(s * M, M)], lsem.at[3]) for s in (1, 2, 3)]
            rest2 = [pltpu.make_async_copy(rt_h, rtv, lsem.at[4]),
                     pltpu.make_async_copy(s_h, sv, lsem.at[4])]
            for c in rest + rest2: c.start()
            lane = lax.broadcasted_iota(i32, (8, N), 1)
            row = lax.broadcasted_iota(i32, (8, N), 0)
            kk = (0x0312 >> ((row >> 1) * 4)) & 3
            word = (((me + kk) & 3) << 1) + (row & 1)
            inword = (lane >> 5) == word
            bit = ((0x8000 >> (lane & 15)) + 0x10000).astype(f32)
            whi = jnp.where(inword & ((lane & 16) == 0), bit, 0.0)
            wlo = jnp.where(inword & ((lane & 16) != 0), bit, 0.0)
            mark("t0_issued")
            cp["i"].wait()
            mark("t1_idx")
            ex = jnp.broadcast_to(iv[...] & 7, (8, N))
            masks, counts = [], []
            for e in range(EL):
                hit = ex == me * EL + e
                hi = jnp.sum(jnp.where(hit, whi, 0.0), axis=1, keepdims=True).astype(i32)
                lo = jnp.sum(jnp.where(hit, wlo, 0.0), axis=1, keepdims=True).astype(i32)
                mv = (hi << 16) | (lo & 0xFFFF)
                cv = (hi >> 16) + (lo >> 16)
                masks.append([mv[r, 0] for r in range(8)])
                counts.append([cv[r, 0] for r in range(8)])
            total = sum(counts[0][:6]) + sum(counts[1][:6])
            chosen = jnp.where(me < 2, ex[:, :128], ex[:, 128:]) == row[:, :128]

            def send_rows(e, r):
                src = sbuf[e][r >> 1]
                def step(_, c):
                    m, pos = c
                    j = lax.clz(m)
                    pos = pos + j
                    m = (m << j) & 0x7FFFFFFF
                    if r < 6:
                        kw = dict(device_id=peer[r >> 1], device_id_type=pl.DeviceIdType.LOGICAL) if logical else dict(device_id=(peer[r >> 1],), device_id_type=MESH)
                        pltpu.make_async_remote_copy(src.at[pl.ds(pos, 1)], rbuf.at[pl.ds(pos, 1)], ssem, rsem, **kw).start()
                    else:
                        pltpu.make_async_copy(src.at[pl.ds(pos, 1)], rbuf.at[pl.ds(pos, 1)], rsem).start()
                    return m, pos
                lax.fori_loop(0, counts[e][r], step, (masks[e][r], i32((r & 1) * 32)))

            def expert(e, s0, ns, split=1):
                w = wv[e].astype(bf16)
                if split == 1:
                    y = _pack(jnp.dot(xv[pl.ds(s0 * M, ns * M), :].astype(bf16), w, preferred_element_type=f32))
                    for s in range(ns):
                        sbuf[e][s0 + s][...] = y[s * M:(s + 1) * M]
                else:
                    c = M // split
                    for p in range(split):
                        sbuf[e][s0][pl.ds(p * c, c), :] = _pack(jnp.dot(xv[pl.ds(s0 * M + p * c, c), :].astype(bf16), w, preferred_element_type=f32))

            mark("t2_masks")
            cp["w0"].wait(); cp["x"].wait()
            mark("t3_w0")
            if fused:
                cp["w1"].wait()
                expert(0, 0, 1); expert(1, 0, 1)
                mark("t4_mm0")
                pl.semaphore_wait(bar, NDEV - 1)
                mark("t5_bar")
                for r in (0, 1): send_rows(0, r)
            else:
                expert(0, 0, 1, split)
                mark("t4_mm0")
                pl.semaphore_wait(bar, NDEV - 1)
                mark("t5_bar")
                for r in (0, 1): send_rows(0, r)
                mark("t6_s0")
                cp["w1"].wait()
                mark("t7_w1")
                expert(1, 0, 1, split)
                mark("t8_mm1")
            for r in (0, 1): send_rows(1, r)
            mark("t9_s1")
            for s in range(3):
                pl.semaphore_signal(done, inc=1, device_id=(peer[s],), device_id_type=MESH)
            for c in rest: c.wait()
            for e in range(EL): expert(e, 1, 3 if selfmm == "with" else 2)
            mark("u0_mmn")
            for r in (2, 3):
                for e in range(EL):
                    send_rows(e, r); send_rows(e, r + 2)
            mark("u1_sn")
            for c in rest2: c.wait()
            xm = xv[pl.ds(3 * M, M), :]
            x_hi = xm.astype(bf16)
            x_lo = (xm - x_hi.astype(f32)).astype(bf16)
            rt = rtv[...]
            r_hi = rt.astype(bf16).astype(f32)
            r2 = jnp.concatenate([r_hi, rt - r_hi], axis=0).astype(bf16)
            s1 = lax.dot_general(r2, jnp.concatenate([x_hi, x_hi], axis=0), NT, preferred_element_type=f32)
            s2 = lax.dot_general(r2, jnp.concatenate([x_lo, x_lo], axis=0), NT, preferred_element_type=f32)
            sc = s1[:8] + (s1[8:] + s2[:8])
            shared = jnp.dot(x_hi, sv[...].astype(bf16), preferred_element_type=f32)
            if selfmm != "with":
                for e in range(EL): expert(e, 3, 1)
            p = jnp.exp(sc - jnp.max(sc, axis=0, keepdims=True))
            gate = jnp.sum(jnp.where(chosen, p, 0.0), axis=0, keepdims=True) / jnp.sum(p, axis=0, keepdims=True)
            diag = lax.broadcasted_iota(i32, (M, 128), 1) == lax.broadcasted_iota(i32, (M, 128), 0) + (me & 1) * M
            g = jnp.broadcast_to(jnp.sum(jnp.where(diag, gate, 0.0), axis=1, keepdims=True), (M, 128))
            mark("u2_gate")
            for r in (6, 7):
                for e in range(EL): send_rows(e, r)
            mark("u3_self")
            def drain(trips, per):
                @pl.loop(0, trips)
                def _(p):
                    for _ in range(per):
                        pltpu.make_async_remote_copy(sbuf[0][0].at[pl.ds(0, 1)], rbuf.at[pl.ds(0, 1)], ssem, rsem,
                                                     device_id=(me,), device_id_type=MESH).wait_send()
            drain(total >> 4, 16); drain((total >> 2) & 3, 4); drain(total & 3, 1)
            mark("u4_drain")
            pl.semaphore_wait(done, NDEV - 1)
            mark("u5_done")
            pltpu.make_async_copy(rbuf, rbuf, rsem).wait()
            mark("u6_recv")
            w = rbuf[...]
            o_ref[:, :128] = shared[:, :128] + g * lax.bitcast_convert_type(w << 16, f32)
            o_ref[:, 128:] = shared[:, 128:] + g * lax.bitcast_convert_type(w & u32(0xFFFF0000), f32)
        pl.run_scoped(scoped,
            pltpu.VMEM((N, D), f32), pltpu.VMEM((EL, D, H), f32), pltpu.VMEM((D, H), f32),
            pltpu.VMEM((8, D), f32), pltpu.VMEM((1, N), i32),
            [[pltpu.VMEM((M, 128), u32)] * NDEV] * EL, pltpu.VMEM((M, 128), u32),
            pltpu.SemaphoreType.DMA((5,)), pltpu.SemaphoreType.DMA, pltpu.SemaphoreType.DMA, pltpu.SemaphoreType.REGULAR)
    hbm = pl.BlockSpec(memory_space=pltpu.HBM)
    return pl.pallas_call(body, out_shape=jax.ShapeDtypeStruct((M, H), f32), in_specs=[hbm] * 5,
        out_specs=pl.BlockSpec(memory_space=pltpu.VMEM),
        compiler_params=pltpu.CompilerParams(collective_id=0),
    )(x, router_W.T, route_idx.reshape(1, N), expert_W, shared_W)
  return kern

pallas_dist_moe_shared_ep_outshard_n256_d128_e2_h256_kernel = make(selfmm='after')
```

```python
import jax
import jax.numpy as jnp
from jax import lax
from jax.experimental import pallas as pl
from jax.experimental.pallas import tpu as pltpu

N_DEV = 4
N_EXP = 8
E_LOC = N_EXP // N_DEV
M = 64
N = N_DEV * M
D = 128
H = 256
LANES = 128
WORD = 32

RING_OFFSET = (2, 1, 3, 0)
FAR, OWN = 0, 3

F32, BF16, I32, U32 = jnp.float32, jnp.bfloat16, jnp.int32, jnp.uint32
MESH = pl.DeviceIdType.MESH


def _matmul(a, b):
    return jnp.dot(a.astype(BF16), b.astype(BF16), preferred_element_type=F32)


def _pack_bf16(y):
    lo, hi = (
        lax.bitcast_convert_type(half.astype(BF16).astype(F32), U32)
        for half in (y[:, :LANES], y[:, LANES:])
    )
    return (lo >> 16) | hi


def _unpack_bf16(w):
    return (
        lax.bitcast_convert_type(w << 16, F32),
        lax.bitcast_convert_type(w & U32(0xFFFF0000), F32),
    )


def _bitmask_weights(me):
    tok = lax.broadcasted_iota(I32, (2 * N_DEV, N), 1)
    r = lax.broadcasted_iota(I32, (2 * N_DEV, N), 0)
    offsets = sum(k << (4 * s) for s, k in enumerate(RING_OFFSET))
    chip = (me + (offsets >> ((r >> 1) * 4))) & (N_DEV - 1)
    in_word = (tok >> 5) == 2 * chip + (r & 1)
    weight = ((0x8000 >> (tok & 15)) + 0x10000).astype(F32)
    return (
        jnp.where(in_word & ((tok & 16) == 0), weight, 0.0),
        jnp.where(in_word & ((tok & 16) != 0), weight, 0.0),
    )


def _bitmasks(hit, weights):
    hi, lo = (
        jnp.sum(jnp.where(hit, w, 0.0), axis=1, keepdims=True).astype(I32)
        for w in weights
    )
    return (hi << 16) | (lo & 0xFFFF), (hi >> 16) + (lo >> 16)


def _gate(x, router_t, chosen, lane0):
    x_hi = x.astype(BF16)
    x_lo = (x - x_hi.astype(F32)).astype(BF16)
    r_hi = router_t.astype(BF16).astype(F32)
    r_hi_lo = jnp.concatenate([r_hi, router_t - r_hi], axis=0).astype(BF16)
    s_hi, s_lo = (
        lax.dot_general(
            r_hi_lo,
            jnp.concatenate([part, part], axis=0),
            (((1,), (1,)), ((), ())),
            preferred_element_type=F32,
        )
        for part in (x_hi, x_lo)
    )
    scores = s_hi[:N_EXP] + (s_hi[N_EXP:] + s_lo[:N_EXP])
    p = jnp.exp(scores - jnp.max(scores, axis=0, keepdims=True))
    picked = jnp.sum(jnp.where(chosen, p, 0.0), axis=0, keepdims=True)
    gate = picked / jnp.sum(p, axis=0, keepdims=True)
    lane = lax.broadcasted_iota(I32, (M, LANES), 1)
    row = lax.broadcasted_iota(I32, (M, LANES), 0)
    column = jnp.sum(jnp.where(lane == row + lane0, gate, 0.0), axis=1, keepdims=True)
    return jnp.broadcast_to(column, (M, LANES))


def _moe_body(
    x_hbm,
    router_hbm,
    idx_hbm,
    w_hbm,
    shared_hbm,
    out_ref,
    x_ref,
    router_ref,
    idx_ref,
    w_ref,
    shared_ref,
    far_bufs,
    near_bufs,
    recv_buf,
    load_sems,
    send_sem,
    recv_sem,
    started_sem,
):
    me = lax.axis_index("i")
    chips = [(me + k) % N_DEV for k in RING_OFFSET]

    def signal_others(sem):
        for chip in chips[:OWN]:
            pl.semaphore_signal(sem, inc=1, device_id=(chip,), device_id_type=MESH)

    def start_loads(group, *pairs):
        copies = [pltpu.make_async_copy(s, d, load_sems.at[group]) for s, d in pairs]
        for copy in copies:
            copy.start()
        return copies

    def wait(copies):
        for copy in copies:
            copy.wait()

    def x_block(s):
        rows = pl.ds(pl.multiple_of(chips[s] * M, M), M)
        return x_hbm.at[rows], x_ref.at[pl.ds(s * M, M)]

    def row_copy(src, slot, pos):
        src, dst = src.at[pl.ds(pos, 1)], recv_buf.at[pl.ds(pos, 1)]
        if slot == OWN:
            return pltpu.make_async_copy(src, dst, recv_sem)
        return pltpu.make_async_remote_copy(
            src, dst, send_sem, recv_sem, device_id=(chips[slot],), device_id_type=MESH
        )

    def send_rows(src, r, mask, count):
        def step(_, carry):
            mask, pos = carry
            skip = lax.clz(mask)
            pos = pos + skip
            mask = (mask << skip) & 0x7FFFFFFF
            row_copy(src, r // 2, pos).start()
            return mask, pos

        lax.fori_loop(0, count, step, (mask, I32(r % 2 * WORD)))

    load_idx = start_loads(0, (idx_hbm, idx_ref))
    load_w0 = start_loads(1, (w_hbm.at[0], w_ref.at[0]))
    barrier = pltpu.get_barrier_semaphore()
    signal_others(barrier)
    load_w0 += start_loads(1, x_block(FAR))
    load_w1 = start_loads(2, (w_hbm.at[1], w_ref.at[1]))
    load_x = start_loads(3, *(x_block(s) for s in range(1, N_DEV)))
    load_own = start_loads(4, (router_hbm, router_ref), (shared_hbm, shared_ref))

    weights = _bitmask_weights(me)
    wait(load_idx)
    expert = jnp.broadcast_to(idx_ref[...] & (N_EXP - 1), (N_EXP, N))
    masks, counts = zip(
        *(_bitmasks(expert == E_LOC * me + e, weights) for e in range(E_LOC))
    )
    far = [[(masks[e][r, 0], counts[e][r, 0]) for r in (0, 1)] for e in range(E_LOC)]
    either, either_count = masks[0] | masks[1], counts[0] + counts[1]
    near = {r: (either[r, 0], either_count[r, 0]) for r in range(2, 2 * N_DEV)}
    n_sent = sum(c for per_expert in far for _, c in per_expert)
    n_sent += sum(near[r][1] for r in range(2, 2 * OWN))
    second_expert = jnp.broadcast_to(masks[1], (2 * N_DEV, H))
    own_half = jnp.where(me < 2, expert[:, :LANES], expert[:, LANES:])
    chosen = own_half == lax.broadcasted_iota(I32, (N_EXP, LANES), 0)

    def compute_far(e):
        for lo in (0, WORD):
            rows = pl.ds(lo, WORD)
            far_bufs[e][rows, :] = _pack_bf16(_matmul(x_ref[rows, :], w_ref[e]))

    def compute_near(first, n_slots):
        x = x_ref[pl.ds(first * M, n_slots * M), :]
        y0, y1 = (_matmul(x, w_ref[e]) for e in range(E_LOC))
        bit = lax.broadcasted_iota(I32, (WORD, H), 0)
        for k in range(2 * n_slots):
            r, rows = 2 * first + k, slice(k * WORD, (k + 1) * WORD)
            y = jnp.where((second_expert[r : r + 1] << bit) < 0, y1[rows], y0[rows])
            near_bufs[r // 2 - 1][pl.ds(r % 2 * WORD, WORD), :] = _pack_bf16(y)

    def send_near(*words):
        for r in words:
            send_rows(near_bufs[r // 2 - 1], r, *near[r])

    wait(load_w0)
    compute_far(0)
    pl.semaphore_wait(barrier, N_DEV - 1)
    for r in (0, 1):
        send_rows(far_bufs[0], r, *far[0][r])
    wait(load_w1)
    compute_far(1)
    for r in (0, 1):
        send_rows(far_bufs[1], r, *far[1][r])

    wait(load_x)
    compute_near(1, 2)
    signal_others(started_sem)
    send_near(2, 4, 3, 5)

    wait(load_own)
    x_own = x_ref[pl.ds(OWN * M, M), :]
    gate = _gate(x_own, router_ref[...], chosen, (me % 2) * M)
    compute_near(OWN, 1)
    shared = _matmul(x_own, shared_ref[...])
    send_near(6, 7)

    for trips, batch in ((n_sent >> 4, 16), ((n_sent >> 2) & 3, 4), (n_sent & 3, 1)):

        @pl.loop(0, trips)
        def _(_, batch=batch):
            for _ in range(batch):
                row_copy(far_bufs[0], FAR, 0).wait_send()

    pl.semaphore_wait(started_sem, N_DEV - 1)
    pltpu.make_async_copy(recv_buf, recv_buf, recv_sem).wait()
    lo, hi = _unpack_bf16(recv_buf[...])
    out_ref[:, :LANES] = shared[:, :LANES] + gate * lo
    out_ref[:, LANES:] = shared[:, LANES:] + gate * hi


def _kernel_body(*refs):
    pl.run_scoped(
        lambda *sems: _moe_body(*refs, *sems),
        pltpu.SemaphoreType.DMA((5,)),
        pltpu.SemaphoreType.DMA,
        pltpu.SemaphoreType.DMA,
        pltpu.SemaphoreType.REGULAR,
    )


def pallas_dist_moe_shared_ep_outshard_n256_d128_e2_h256_kernel(
    x: jax.Array,
    router_W: jax.Array,
    route_idx: jax.Array,
    expert_W: jax.Array,
    shared_W: jax.Array,
):
    rows = pltpu.VMEM((M, LANES), U32)
    return pl.pallas_call(
        _kernel_body,
        out_shape=jax.ShapeDtypeStruct((M, H), F32),
        in_specs=[pl.BlockSpec(memory_space=pltpu.HBM)] * 5,
        out_specs=pl.BlockSpec(memory_space=pltpu.VMEM),
        scratch_shapes=[
            pltpu.VMEM((N, D), F32),
            pltpu.VMEM((N_EXP, D), F32),
            pltpu.VMEM((1, N), I32),
            pltpu.VMEM((E_LOC, D, H), F32),
            pltpu.VMEM((D, H), F32),
            [rows] * E_LOC,
            [rows] * (N_DEV - 1),
            rows,
        ],
        compiler_params=pltpu.CompilerParams(collective_id=0),
    )(x, router_W.T, route_idx.reshape(1, N), expert_W, shared_W)
```

```python
import jax
import jax.numpy as jnp
from jax import lax
from jax.experimental import pallas as pl
from jax.experimental.pallas import tpu as pltpu

N_DEV = 4
N_EXP = 8
E_LOC = N_EXP // N_DEV
M = 64
N = N_DEV * M
D = 128
H = 256
LANES = 128
WORD = 32

RING_OFFSET = (2, 1, 3, 0)
FAR, OWN = 0, 3

F32, BF16, I32, U32 = jnp.float32, jnp.bfloat16, jnp.int32, jnp.uint32
MESH = pl.DeviceIdType.MESH


def _matmul(a, b):
    return jnp.dot(a.astype(BF16), b.astype(BF16), preferred_element_type=F32)


def _pack_bf16(y):
    lo, hi = (
        lax.bitcast_convert_type(half.astype(BF16).astype(F32), U32)
        for half in (y[:, :LANES], y[:, LANES:])
    )
    return (lo >> 16) | hi


def _unpack_bf16(w):
    return (
        lax.bitcast_convert_type(w << 16, F32),
        lax.bitcast_convert_type(w & U32(0xFFFF0000), F32),
    )


def _bitmask_weights(me):
    tok = lax.broadcasted_iota(I32, (2 * N_DEV, N), 1)
    r = lax.broadcasted_iota(I32, (2 * N_DEV, N), 0)
    offsets = sum(k << (4 * s) for s, k in enumerate(RING_OFFSET))
    chip = (me + (offsets >> ((r >> 1) * 4))) & (N_DEV - 1)
    in_word = (tok >> 5) == 2 * chip + (r & 1)
    weight = ((0x8000 >> (tok & 15)) + 0x10000).astype(F32)
    return (
        jnp.where(in_word & ((tok & 16) == 0), weight, 0.0),
        jnp.where(in_word & ((tok & 16) != 0), weight, 0.0),
    )


def _bitmasks(hit, weights):
    hi, lo = (
        jnp.sum(jnp.where(hit, w, 0.0), axis=1, keepdims=True).astype(I32)
        for w in weights
    )
    return (hi << 16) | (lo & 0xFFFF), (hi >> 16) + (lo >> 16)


def _gate(x, router_t, chosen, lane0):
    x_hi = x.astype(BF16)
    x_lo = (x - x_hi.astype(F32)).astype(BF16)
    r_hi = router_t.astype(BF16).astype(F32)
    r_hi_lo = jnp.concatenate([r_hi, router_t - r_hi], axis=0).astype(BF16)
    s_hi, s_lo = (
        lax.dot_general(
            r_hi_lo,
            jnp.concatenate([part, part], axis=0),
            (((1,), (1,)), ((), ())),
            preferred_element_type=F32,
        )
        for part in (x_hi, x_lo)
    )
    scores = s_hi[:N_EXP] + (s_hi[N_EXP:] + s_lo[:N_EXP])
    p = jnp.exp(scores - jnp.max(scores, axis=0, keepdims=True))
    picked = jnp.sum(jnp.where(chosen, p, 0.0), axis=0, keepdims=True)
    gate = picked / jnp.sum(p, axis=0, keepdims=True)
    lane = lax.broadcasted_iota(I32, (M, LANES), 1)
    row = lax.broadcasted_iota(I32, (M, LANES), 0)
    column = jnp.sum(jnp.where(lane == row + lane0, gate, 0.0), axis=1, keepdims=True)
    return jnp.broadcast_to(column, (M, LANES))


def _moe_body(
    x_hbm,
    router_hbm,
    idx_hbm,
    w_hbm,
    shared_hbm,
    out_ref,
    x_ref,
    router_ref,
    idx_ref,
    w_ref,
    shared_ref,
    far_bufs,
    near_bufs,
    recv_buf,
    load_sems,
    send_sem,
    recv_sem,
    started_sem,
):
    me = lax.axis_index("i")
    chips = [(me + k) & (N_DEV - 1) for k in RING_OFFSET]

    def signal_others(sem):
        for chip in chips[:OWN]:
            pl.semaphore_signal(sem, inc=1, device_id=(chip,), device_id_type=MESH)

    def start_loads(group, *pairs):
        copies = [pltpu.make_async_copy(s, d, load_sems.at[group]) for s, d in pairs]
        for copy in copies:
            copy.start()
        return copies

    def wait(copies):
        for copy in copies:
            copy.wait()

    def x_block(s):
        rows = pl.ds(pl.multiple_of(chips[s] * M, M), M)
        return x_hbm.at[rows], x_ref.at[pl.ds(s * M, M)]

    def row_copy(src, slot, pos):
        src, dst = src.at[pl.ds(pos, 1)], recv_buf.at[pl.ds(pos, 1)]
        if slot == OWN:
            return pltpu.make_async_copy(src, dst, recv_sem)
        return pltpu.make_async_remote_copy(
            src, dst, send_sem, recv_sem, device_id=(chips[slot],), device_id_type=MESH
        )

    def send_rows(src, r, mask, count):
        def step(_, carry):
            mask, pos = carry
            skip = lax.clz(mask)
            pos = pos + skip
            mask = (mask << skip) & 0x7FFFFFFF
            row_copy(src, r // 2, pos).start()
            return mask, pos

        lax.fori_loop(0, count, step, (mask, I32(r % 2 * WORD)))

    load_idx = start_loads(0, (idx_hbm, idx_ref))
    load_w0 = start_loads(1, (w_hbm.at[0], w_ref.at[0]), x_block(FAR))
    load_w1 = start_loads(2, (w_hbm.at[1], w_ref.at[1]))
    barrier = pltpu.get_barrier_semaphore()
    signal_others(barrier)
    load_x = start_loads(3, *(x_block(s) for s in range(1, N_DEV)))
    load_own = start_loads(4, (router_hbm, router_ref), (shared_hbm, shared_ref))

    weights = _bitmask_weights(me)
    wait(load_idx)
    expert = jnp.broadcast_to(idx_ref[...] & (N_EXP - 1), (N_EXP, N))
    masks, counts = zip(
        *(_bitmasks(expert == E_LOC * me + e, weights) for e in range(E_LOC))
    )
    far = [[(masks[e][r, 0], counts[e][r, 0]) for r in (0, 1)] for e in range(E_LOC)]
    either, either_count = masks[0] | masks[1], counts[0] + counts[1]
    near = {r: (either[r, 0], either_count[r, 0]) for r in range(2, 2 * N_DEV)}
    n_sent = sum(c for per_expert in far for _, c in per_expert)
    n_sent += sum(near[r][1] for r in range(2, 2 * OWN))
    second_expert = jnp.broadcast_to(masks[1], (2 * N_DEV, H))
    own_half = jnp.where(me < 2, expert[:, :LANES], expert[:, LANES:])
    chosen = own_half == lax.broadcasted_iota(I32, (N_EXP, LANES), 0)

    def compute_far(e):
        for lo in (0, WORD):
            rows = pl.ds(lo, WORD)
            far_bufs[e][rows, :] = _pack_bf16(_matmul(x_ref[rows, :], w_ref[e]))

    def compute_near(first, n_slots):
        x = x_ref[pl.ds(first * M, n_slots * M), :]
        y0, y1 = (_matmul(x, w_ref[e]) for e in range(E_LOC))
        bit = lax.broadcasted_iota(I32, (WORD, H), 0)
        for k in range(2 * n_slots):
            r, rows = 2 * first + k, slice(k * WORD, (k + 1) * WORD)
            y = jnp.where((second_expert[r : r + 1] << bit) < 0, y1[rows], y0[rows])
            near_bufs[r // 2 - 1][pl.ds(r % 2 * WORD, WORD), :] = _pack_bf16(y)

    def send_near(*words):
        for r in words:
            send_rows(near_bufs[r // 2 - 1], r, *near[r])

    wait(load_w0)
    compute_far(0)
    pl.semaphore_wait(barrier, N_DEV - 1)
    for r in (0, 1):
        send_rows(far_bufs[0], r, *far[0][r])
    wait(load_w1)
    compute_far(1)
    for r in (0, 1):
        send_rows(far_bufs[1], r, *far[1][r])

    wait(load_x)
    compute_near(1, 2)
    signal_others(started_sem)
    send_near(2, 4, 3, 5)

    wait(load_own)
    x_own = x_ref[pl.ds(OWN * M, M), :]
    gate = _gate(x_own, router_ref[...], chosen, (me & 1) * M)
    compute_near(OWN, 1)
    shared = _matmul(x_own, shared_ref[...])
    send_near(6, 7)

    for trips, batch in ((n_sent >> 4, 16), ((n_sent >> 2) & 3, 4), (n_sent & 3, 1)):

        @pl.loop(0, trips)
        def _(_, batch=batch):
            for _ in range(batch):
                row_copy(far_bufs[0], FAR, 0).wait_send()

    pl.semaphore_wait(started_sem, N_DEV - 1)
    pltpu.make_async_copy(recv_buf, recv_buf, recv_sem).wait()
    lo, hi = _unpack_bf16(recv_buf[...])
    out_ref[:, :LANES] = shared[:, :LANES] + gate * lo
    out_ref[:, LANES:] = shared[:, LANES:] + gate * hi


def _kernel_body(*refs):
    pl.run_scoped(
        lambda *sems: _moe_body(*refs, *sems),
        pltpu.SemaphoreType.DMA((5,)),
        pltpu.SemaphoreType.DMA,
        pltpu.SemaphoreType.DMA,
        pltpu.SemaphoreType.REGULAR,
    )


def pallas_dist_moe_shared_ep_outshard_n256_d128_e2_h256_kernel(
    x: jax.Array,
    router_W: jax.Array,
    route_idx: jax.Array,
    expert_W: jax.Array,
    shared_W: jax.Array,
):
    rows = pltpu.VMEM((M, LANES), U32)
    return pl.pallas_call(
        _kernel_body,
        out_shape=jax.ShapeDtypeStruct((M, H), F32),
        in_specs=[pl.BlockSpec(memory_space=pltpu.HBM)] * 5,
        out_specs=pl.BlockSpec(memory_space=pltpu.VMEM),
        scratch_shapes=[
            pltpu.VMEM((N, D), F32),
            pltpu.VMEM((N_EXP, D), F32),
            pltpu.VMEM((1, N), I32),
            pltpu.VMEM((E_LOC, D, H), F32),
            pltpu.VMEM((D, H), F32),
            [rows] * E_LOC,
            [rows] * (N_DEV - 1),
            rows,
        ],
        compiler_params=pltpu.CompilerParams(collective_id=0),
    )(x, router_W.T, route_idx.reshape(1, N), expert_W, shared_W)
```
